```python
import numpy as np

kernel_name = "dist_max_ax1_xy_m4096_n1024"

def setup_inputs():
    return {"x": np.random.randn(8192, 2048).astype(np.float32)}

def reference(x: np.ndarray) -> np.ndarray:
    return np.max(x, axis=1, keepdims=True)
```

```python
import functools

import jax
import jax.numpy as jnp
from jax import lax
from jax.experimental import pallas as pl
from jax.experimental.pallas import tpu as pltpu

_ROWS, _COLS = 4096, 1024
_TILES = 4096
_STREAM_TILES = 128
_CHUNK_TILES = 16
_STREAMS = 16
_HALF_STEPS = _STREAM_TILES // _CHUNK_TILES
_STEPS = 2 * _HALF_STEPS
_LAST = _STEPS - 1

_SKEW = 9
_PREFILL = 25
_AHEAD = 4
_GROUPS = ((0, 8), (8, 14), (14, 16))


def _row_max_kernel(x_ref, o_ref, buf, load_sems, send_sems, recv_sems, *messages):
    mine, theirs = messages[: len(_GROUPS)], messages[len(_GROUPS) :]

    def start_step(t, sem_of, first_step=False):
        half_start = (t >> 3) * (_STREAMS * _STREAM_TILES)
        base = half_start + (t & 7) * _CHUNK_TILES - _SKEW
        started = 0
        for u in range(_STREAMS // 2):
            for offset in (0, 8):
                for queue in range(2):
                    s = queue * (_STREAMS // 2) + u
                    src = base + s * _STREAM_TILES + offset
                    dst = s * _CHUNK_TILES + offset
                    parts = [(src, dst, 8)]
                    if first_step and src + 8 <= 0:
                        parts = [(src + _TILES, dst, 8)]
                    elif first_step and src < 0:
                        parts = [(0, dst - src, 8 + src), (src + _TILES, dst, -src)]
                    for a, b, n in parts:
                        prefill = first_step and started < _PREFILL
                        pltpu.make_async_copy(
                            x_ref.at[pl.ds(a, n)], buf.at[t, pl.ds(b, n)], sem_of(s)
                        ).start(priority=1 if prefill else queue)
                        started += 1

    def wait_filled(view, sem):
        pltpu.make_async_copy(view, view, sem).wait()

    def tiles_max(t, first, n):
        vs = [buf[t, first + k] for k in range(n)]
        while len(vs) > 1:
            pairs = [jnp.maximum(a, b) for a, b in zip(vs[::2], vs[1::2])]
            vs = pairs + vs[2 * len(pairs) :]
        return vs[0]

    lane = lax.broadcasted_iota(jnp.int32, (8, 128), 1)
    sublane = lax.broadcasted_iota(jnp.int32, (8, 128), 0)
    diagonal = lane - sublane

    def place(block, j, acc):
        return jnp.where(diagonal == 8 * j, jnp.max(block, axis=1, keepdims=True), acc)

    head = _SKEW - 8

    def fold(t, s, carry, acc):
        first, j = s * _CHUNK_TILES, (t & 7) * 2
        acc = place(jnp.maximum(carry, tiles_max(t, first, head)), j - 2, acc)
        acc = place(tiles_max(t, first + head, 8), j - 1, acc)
        return tiles_max(t, first + _SKEW, _CHUNK_TILES - _SKEW), acc

    def next_stream(row):
        row = (row + 1) % (2 * _STREAMS)
        return row // _STREAMS * _HALF_STEPS, row % _STREAMS * _CHUNK_TILES

    def fold_block15(row, acc):
        t, first = next_stream(row)
        return place(tiles_max(t, first + head, 8), 15, acc)

    def finish(row, carry, acc):
        t, first = next_stream(row)
        acc = place(jnp.maximum(carry, tiles_max(t, first, head)), 14, acc)
        return jnp.max(acc, axis=0, keepdims=True)

    def step(t, state, prefetch):
        wait_filled(buf.at[t], load_sems.at[t])
        state = tuple(fold(t, s, *state[s]) for s in range(_STREAMS))
        if prefetch:
            start_step(t + _AHEAD, lambda s: load_sems.at[t + _AHEAD])
        return state

    start_step(0, lambda s: load_sems.at[0], first_step=True)

    @pl.loop(1, _AHEAD)
    def _(t):
        start_step(t, lambda s: load_sems.at[t])

    peer = (lax.axis_index("x"), 1 - lax.axis_index("y"))
    barrier = pltpu.get_barrier_semaphore()
    pl.semaphore_signal(
        barrier, inc=1, device_id=peer, device_id_type=pl.DeviceIdType.MESH
    )

    lowest = jnp.full((8, 128), -jnp.inf, jnp.float32)
    empty = ((lowest, lowest),) * _STREAMS
    step_ahead = functools.partial(step, prefetch=True)
    first_half = lax.fori_loop(0, _HALF_STEPS, step_ahead, empty)
    state = lax.fori_loop(_HALF_STEPS, _LAST - _AHEAD, step_ahead, empty)
    start_step(
        _LAST, lambda s: load_sems.at[_LAST + sum(s >= end for _, end in _GROUPS)]
    )

    for row, (carry, acc) in enumerate(first_half):
        mine[0][row : row + 1, :] = finish(row, carry, fold_block15(row, acc))
    state = tuple(
        (carry, fold_block15(_STREAMS + s, acc)) for s, (carry, acc) in enumerate(state)
    )
    state = lax.fori_loop(
        _LAST - _AHEAD, _LAST, functools.partial(step, prefetch=False), state
    )

    pl.semaphore_wait(barrier, 1)
    copies = []
    for k, (begin, end) in enumerate(_GROUPS):
        tiles = pl.ds(begin * _CHUNK_TILES, (end - begin) * _CHUNK_TILES)
        wait_filled(buf.at[_LAST, tiles], load_sems.at[_LAST + k])
        for s in range(begin, end):
            r = mine[k].shape[0] - (end - s)
            mine[k][r : r + 1, :] = finish(_STREAMS + s, *fold(_LAST, s, *state[s]))
        copy = pltpu.make_async_remote_copy(
            src_ref=mine[k],
            dst_ref=theirs[k],
            send_sem=send_sems.at[k],
            recv_sem=recv_sems.at[k],
            device_id=peer,
            device_id_type=pl.DeviceIdType.MESH,
        )
        copy.start()
        copies.append(copy)

    for copy in copies:
        copy.wait_send()
    row = 0
    for k, copy in enumerate(copies):
        own = mine[k][...]
        copy.wait_recv()
        o_ref[row : row + own.shape[0], :] = jnp.maximum(own, theirs[k][...])
        row += own.shape[0]


def pallas_dist_max_ax1_xy_m4096_n1024_kernel(x: jax.Array):
    assert x.shape == (_ROWS, _COLS) and x.dtype == jnp.float32
    tiles = x.reshape(_ROWS // 8, 8, _COLS // 128, 128).transpose(0, 2, 1, 3)
    tiles = tiles.reshape(_TILES, 8, 128)
    messages = [
        pltpu.VMEM((end - begin + (_STREAMS if k == 0 else 0), 128), jnp.float32)
        for k, (begin, end) in enumerate(_GROUPS)
    ]
    out = pl.pallas_call(
        _row_max_kernel,
        out_shape=jax.ShapeDtypeStruct((_ROWS // 128, 128), jnp.float32),
        in_specs=[pl.BlockSpec(memory_space=pltpu.MemorySpace.HBM)],
        out_specs=pl.BlockSpec(memory_space=pltpu.MemorySpace.VMEM),
        scratch_shapes=[
            pltpu.VMEM((_STEPS, _STREAMS * _CHUNK_TILES, 8, 128), jnp.float32),
            pltpu.SemaphoreType.DMA((_LAST + len(_GROUPS),)),
            pltpu.SemaphoreType.DMA((len(_GROUPS),)),
            pltpu.SemaphoreType.DMA((len(_GROUPS),)),
            *messages,
            *messages,
        ],
        compiler_params=pltpu.CompilerParams(
            collective_id=0,
            vmem_limit_bytes=32 * 1024 * 1024,
            disable_semaphore_checks=True,
        ),
    )(tiles)
    return out.reshape(_ROWS, 1)
```
